```python
import numpy as np

kernel_name = "dist_embed_lookup_i_n2048_v16384_d1024"

def setup_inputs():
    table = np.random.randn(65536, 1024).astype(np.float32)
    idx = np.random.randint(0, 65536, size=(2048,)).astype(np.int32)
    return {"table": table, "idx": idx}

def reference(table: np.ndarray, idx: np.ndarray) -> np.ndarray:
    return table[idx]
```

```python
import contextlib
import jax
import jax.numpy as jnp
from jax import lax
from jax.experimental import pallas as pl
from jax.experimental.pallas import tpu as pltpu

N_DEV = 4
N = 2048
V = 16384
D = 1024
H = D // 2
LC = 3
S = 32
LAG = 3
NG = 16
G = 32
FLAG = 1
PROF = 0
MESH = pl.DeviceIdType.MESH
OWN, FROM_R, DIAG, FROM_L = 0, 1, 2, 3


def scope(name):
    return jax.named_scope(name) if PROF else contextlib.nullcontext()


def pallas_dist_embed_lookup_i_n2048_v16384_d1024_kernel(table, idx):
    C = 1 << LC
    NCH = N // C
    M = NCH + 3
    idx2 = idx.reshape(N // 128, 128)

    def body(idx_hbm, idx2_hbm, tab_ref, out_ref,
             idx_s, lst, meta_s, idx_v, meta_v, gbuf, pbuf,
             misc_sem, gsem, ssem, rsem):
        me = lax.axis_index("i")
        left = (me + 3) & 3
        right = (me + 1) & 3

        cp_s = pltpu.make_async_copy(idx_hbm, idx_s, misc_sem.at[0])
        cp_s.start()
        bar = pltpu.get_barrier_semaphore()
        for nb in (left, right):
            pl.semaphore_signal(bar, inc=1, device_id=(nb,), device_id_type=MESH)
        cp_v = pltpu.make_async_copy(idx2_hbm, idx_v, misc_sem.at[1])
        cp_v.start()
        with scope("idxw"):
            cp_s.wait()

        base = me * V

        def chunk_rows(reg, k):
            return pbuf.at[pl.ds(pl.multiple_of(reg * N + k * C, C), C)]

        def rcopy(src_reg, dst_reg, k, tgt, si):
            return pltpu.make_async_remote_copy(
                src_ref=chunk_rows(src_reg, k), dst_ref=chunk_rows(dst_reg, k),
                send_sem=ssem, recv_sem=rsem.at[si],
                device_id=(tgt,), device_id_type=MESH)

        def wait_recv(reg, k, si):
            rcopy(reg, reg, k, me, si).wait_recv()

        def wait_send(_):
            rcopy(OWN, OWN, 0, me, 0).wait_send()

        def issue_gather(k):
            for r in range(C):
                row = lst[k * C + r]
                pltpu.make_async_copy(
                    tab_ref.at[pl.ds(row, 1)],
                    gbuf.at[k, pl.ds(r, 1)], gsem.at[k & (NG - 1)]).start()

        def pack_send(k):
            pltpu.make_async_copy(gbuf.at[k], gbuf.at[k], gsem.at[k & (NG - 1)]).wait()
            x = gbuf[k]
            xb = pltpu.bitcast(x.astype(jnp.bfloat16).astype(jnp.float32), jnp.uint32)
            w = xb[:, :H] | (xb[:, H:] >> 16)
            pbuf[pl.ds(pl.multiple_of(OWN * N + k * C, C), C), :] = w

            @pl.when(k == 0)
            def _():
                with scope("bar"):
                    pl.semaphore_wait(bar, 2)
            rcopy(OWN, FROM_R, k, left, M - 1 - k).start()
            rcopy(OWN, FROM_L, k, right, k).start()

        def loop(lo, hi, fn):
            def b(k, c):
                fn(k)
                return c
            lax.fori_loop(lo, hi, b, 0)

        def step(t, carry):
            cnt, issued, sent = carry
            for i in range(S):
                v = (idx_s[t * S + i] - base) & (N_DEV * V - 1)
                lst[cnt] = v
                cnt = cnt + lax.shift_right_logical(v - V, 31)
            new_issued = cnt >> LC
            loop(issued, new_issued, issue_gather)
            new_sent = jnp.maximum(sent, new_issued - LAG)
            loop(sent, new_sent, pack_send)
            return cnt, new_issued, new_sent

        with scope("phA"):
            cnt, issued, sent = lax.fori_loop(0, N // S, step, (jnp.int32(0),) * 3)
        for i in range(C):
            lst[cnt + i] = 0
        n_me = jnp.maximum((cnt + C - 1) >> LC, 1)
        loop(issued, n_me, issue_gather)

        cp_v.wait()
        rel = ((idx_v[...] >> 14) - me) & 3
        ms = [(rel == o).astype(jnp.float32) for o in range(N_DEV)]
        m = jnp.concatenate(ms, axis=0).astype(jnp.bfloat16)
        ra = lax.broadcasted_iota(jnp.int32, (128, 256), 0)
        rb = lax.broadcasted_iota(jnp.int32, (128, 256), 1)
        rhs = jnp.where((ra < rb), 1.0, 0.0).astype(jnp.bfloat16)
        ee = jnp.dot(m, rhs, preferred_element_type=jnp.float32)
        e = ee[:, :128]
        tot = ee[:, 128:]
        li = lax.broadcasted_iota(jnp.int32, (64, 64), 0)
        lj = lax.broadcasted_iota(jnp.int32, (64, 64), 1)
        lm = jnp.where(((li >> 4) == (lj >> 4)) & (lj < li), 1.0, 0.0).astype(jnp.bfloat16)
        off = jnp.dot(lm, tot.astype(jnp.bfloat16), preferred_element_type=jnp.float32)
        rk = e + off
        slot = ms[0] * rk[0:16]
        for o in range(1, N_DEV):
            slot = slot + ms[o] * (rk[16 * o:16 * o + 16] + float(o * N))
        inc = off + tot
        meta_v[0:16, :] = slot.astype(jnp.int32)
        meta_v[16:32, :] = ((rk[16 * DIAG:16 * DIAG + 16] + ms[DIAG]).astype(jnp.int32) + (C - 1)) >> LC
        sub = lax.broadcasted_iota(jnp.int32, (8, 128), 0)
        tl = jnp.zeros((8, 128), jnp.float32)
        for o in range(N_DEV):
            tl = jnp.where(sub == o, jnp.broadcast_to(inc[16 * o + 15:16 * o + 16], (8, 128)), tl)
        meta_v[32:40, :] = jnp.maximum((tl.astype(jnp.int32) + (C - 1)) >> LC, 1)
        cp_m = pltpu.make_async_copy(meta_v, meta_s, misc_sem.at[2])
        cp_m.start()

        loop(sent, n_me, pack_send)
        with scope("metaw"):
            cp_m.wait()

        n_l, n_r, n_d = meta_s[32 + FROM_L, 0], meta_s[32 + FROM_R, 0], meta_s[32 + DIAG, 0]

        def via_left(k, d):
            return (k < d) | ((k >= jnp.abs(d)) & (((k + d) & 1) == 0))

        def fwd(k, nf):
            f1 = (k < n_l) & via_left(k, n_d - n_me)
            f2 = (k < n_r) & jnp.logical_not(via_left(k, n_me - n_d))

            @pl.when(k < n_l)
            def _():
                wait_recv(FROM_L, k, k)

            @pl.when(f1)
            def _():
                rcopy(FROM_L, DIAG, k, right, n_me + k).start()

            @pl.when(k < n_r)
            def _():
                wait_recv(FROM_R, k, M - 1 - k)

            @pl.when(f2)
            def _():
                rcopy(FROM_R, DIAG, k, left, n_d + k).start()
            return nf + f1.astype(jnp.int32) + f2.astype(jnp.int32)

        with scope("phC"):
            n_f = lax.fori_loop(0, jnp.maximum(n_l, n_r), fwd, jnp.int32(0))
        n_s = n_f + 2 * n_me

        NB = N // 128

        def blk(b, carry):
            have, done = carry
            for g in range(128 // G):
                c0 = g * G
                need = meta_s[16 + b, c0 + G - 1]
                loop(have, need, lambda k: wait_recv(DIAG, k, n_l + k))
                have = need
                rows = [pbuf[pl.ds(meta_s[b, c0 + r], 1), :] for r in range(G)]
                w = jnp.concatenate(rows, axis=0)
                hi = pltpu.bitcast(w & jnp.uint32(0xFFFF0000), jnp.float32)
                lo = pltpu.bitcast(w << 16, jnp.float32)
                p0 = pl.multiple_of(b * 128 + c0, G)
                out_ref[pl.ds(p0, G), 0:H] = hi.astype(out_ref.dtype)
                out_ref[pl.ds(p0, G), H:D] = lo.astype(out_ref.dtype)
                if g == 0:
                    tgt = n_s - ((n_f * (NB - b + FLAG)) >> 4)
                    loop(done, tgt, wait_send)
                    done = jnp.maximum(tgt, done)
            return have, done

        with scope("phD"):
            have, done = lax.fori_loop(0, NB, blk, (jnp.int32(0), jnp.int32(0)))
        loop(have, n_d, lambda k: wait_recv(DIAG, k, n_l + k))
        with scope("fin"):
            loop(done, n_s, wait_send)

    return pl.pallas_call(
        body,
        out_shape=jax.ShapeDtypeStruct((N, D), jnp.bfloat16),
        in_specs=[pl.BlockSpec(memory_space=pl.ANY)] * 3,
        out_specs=pl.BlockSpec(memory_space=pltpu.VMEM),
        scratch_shapes=[
            pltpu.SMEM((N,), jnp.int32),
            pltpu.SMEM((N + C,), jnp.int32),
            pltpu.SMEM((40, 128), jnp.int32),
            pltpu.VMEM((16, 128), jnp.int32),
            pltpu.VMEM((40, 128), jnp.int32),
            pltpu.VMEM((NCH, C, D), jnp.float32),
            pltpu.VMEM((N_DEV * N, H), jnp.uint32),
            pltpu.SemaphoreType.DMA((3,)),
            pltpu.SemaphoreType.DMA((NG,)),
            pltpu.SemaphoreType.DMA,
            pltpu.SemaphoreType.DMA((M,)),
        ],
        compiler_params=pltpu.CompilerParams(
            collective_id=0, vmem_limit_bytes=64 << 20,
            disable_bounds_checks=True, disable_semaphore_checks=True),
    )(idx, idx2, table)
```

```python
import contextlib
import functools
import jax
import jax.numpy as jnp
from jax import lax
from jax.experimental import pallas as pl
from jax.experimental.pallas import tpu as pltpu

N_DEV = 4
N = 2048
V = 16384
D = 1024
H = D // 2
LC = 3
S = 32
LAG = 2
NG = 16
G = 32
FLAG = 1
PROF = 0
I0 = 128
K0 = 3
TL = 6
LAG2 = 2
LAGB = 1
TB = 16
PB0 = 5
MESH = pl.DeviceIdType.MESH
OWN, FROM_R, DIAG, FROM_L = 0, 1, 2, 3


def scope(name):
    return jax.named_scope(name) if PROF else contextlib.nullcontext()


def pallas_dist_embed_lookup_i_n2048_v16384_d1024_kernel(table, idx):
    C = 1 << LC
    NCH = N // C
    M = NCH + 3
    NB = N // 128
    P0 = 128 * PB0
    idx2 = idx.reshape(NB, 128)

    def body(idx_hbm, idx2_hbm, tab_ref, out_ref,
             idx_s, lst, row_s, first_s, slot_s, meta_s,
             idx_v, row_v, first_v, slot_v, meta_v, gbuf, pbuf,
             misc_sem, gsem, ssem, rsem, rdy):
        me = lax.axis_index("i")
        left = (me + 3) & 3
        right = (me + 1) & 3

        cp_s0 = pltpu.make_async_copy(idx_hbm.at[pl.ds(0, I0)], idx_s.at[pl.ds(0, I0)], misc_sem.at[0])
        cp_s0.start()
        bar = pltpu.get_barrier_semaphore()
        is_mid = (me & 1) == 1
        n_bar = jnp.where(is_mid, 1, 2 - me)

        @pl.when(me != 2)
        def _():
            for nb in (left, right):
                pl.semaphore_signal(bar, inc=1, device_id=(nb,), device_id_type=MESH)
        cp_s1 = pltpu.make_async_copy(idx_hbm.at[pl.ds(I0, P0 - I0)], idx_s.at[pl.ds(I0, P0 - I0)], misc_sem.at[1])
        cp_s1.start()
        cp_v = pltpu.make_async_copy(idx2_hbm, idx_v, misc_sem.at[2])
        cp_v.start()
        cp_row = pltpu.make_async_copy(row_v, row_s, misc_sem.at[3])
        cp_first = pltpu.make_async_copy(first_v, first_s, misc_sem.at[4])
        cp_slot = pltpu.make_async_copy(slot_v, slot_s, misc_sem.at[5])
        cp_meta = pltpu.make_async_copy(meta_v, meta_s, misc_sem.at[6])

        @pl.when(me == 2)
        def _():
            with scope("bar2"):
                pl.semaphore_wait(bar, 2)
            for nb in (left, right):
                pl.semaphore_signal(rdy, inc=1, device_id=(nb,), device_id_type=MESH)
        with scope("idxw"):
            cp_s0.wait()

        base = me * V

        def chunk_rows(reg, k, sz):
            return pbuf.at[pl.ds(pl.multiple_of((reg * N + k * C) * 4, 4 * C), 4 * sz)]

        def rcopy(src_reg, dst_reg, k, tgt, si, sz=C):
            return pltpu.make_async_remote_copy(
                src_ref=chunk_rows(src_reg, k, sz), dst_ref=chunk_rows(dst_reg, k, sz),
                send_sem=ssem, recv_sem=rsem.at[si],
                device_id=(tgt,), device_id_type=MESH)

        def wait_recv(reg, k, si, sz=C):
            rcopy(reg, reg, k, me, si, sz).wait_recv()

        def wait_send(_=None, sz=C):
            rcopy(OWN, OWN, 0, me, 0, sz).wait_send()

        def sized(r, fn):
            lax.switch((r >> 1) - 1, [functools.partial(fn, s) for s in range(2, C + 1, 2)])

        def loop(lo, hi, fn):
            def b(k, c):
                fn(k)
                return c
            lax.fori_loop(lo, hi, b, 0)

        def send_l(kk, sz=C):
            rcopy(OWN, FROM_R, kk, left, M - 1 - kk, sz).start()

        def send_r(kk, sz=C):
            rcopy(OWN, FROM_L, kk, right, kk, sz).start()

        def catch_up(n):
            with scope("rdy"):
                pl.semaphore_wait(rdy, 1)

            @pl.when(me == 3)
            def _():
                loop(0, n, send_l)

            @pl.when(me == 1)
            def _():
                loop(0, n, send_r)

        def issue_gather(k):
            for r in range(C):
                row = lst[k * C + r] & (V - 1)
                pltpu.make_async_copy(
                    tab_ref.at[pl.ds(row, 1)],
                    gbuf.at[k, pl.ds(r, 1)], gsem.at[k & (NG - 1)]).start()

        def pack(k):
            pltpu.make_async_copy(gbuf.at[k], gbuf.at[k], gsem.at[k & (NG - 1)]).wait()
            x = gbuf[k]
            xb = pltpu.bitcast(x.astype(jnp.bfloat16).astype(jnp.float32), jnp.uint32)
            w = xb[:, :H] | (xb[:, H:] >> 16)
            for j in range(4):
                pbuf[pl.ds((OWN * N + k * C) * 4 + j, C, stride=4), :] = w[:, 128 * j:128 * (j + 1)]

            @pl.when(k == 0)
            def _():
                with scope("bar"):
                    pl.semaphore_wait(bar, n_bar)

        def pack_send(k):
            pack(k)

            @pl.when((k == K0) & is_mid)
            def _():
                catch_up(K0)

            @pl.when((k >= K0) | (me != 3))
            def _():
                send_l(k)

            @pl.when((k >= K0) | (me != 1))
            def _():
                send_r(k)

        def vector_phase():
            cp_v.wait()
            idxv = idx_v[...] & (N_DEV * V - 1)
            pos = (lax.broadcasted_iota(jnp.int32, (NB, 128), 0) * 128
                   + lax.broadcasted_iota(jnp.int32, (NB, 128), 1))
            sub = lax.broadcasted_iota(jnp.int32, (8, 128), 0)
            idx_t = idxv.T
            rows = {pb: jnp.broadcast_to(idxv[pb:pb + 1, :], (8, 128)) for pb in range(PB0, NB)}
            acc = {pb: jnp.full((8, 128), N, jnp.int32) for pb in range(PB0, NB)}
            for b in range(NB - 1, -1, -1):
                xb = jnp.broadcast_to(idx_t[:, b:b + 1], (128, 128))
                for u in range(15, -1, -1):
                    xq = xb[8 * u:8 * u + 8]
                    qv = sub + (128 * b + 8 * u)
                    for pb in range(max(b, PB0), NB):
                        acc[pb] = jnp.where(xq == rows[pb], qv, acc[pb])
            first = jnp.concatenate(
                [pos[0:PB0]] + [jnp.min(acc[pb], axis=0, keepdims=True) for pb in range(PB0, NB)],
                axis=0)
            rel = jnp.where(first == pos, ((idxv >> 14) - me) & 3, N_DEV)
            row_v[...] = jnp.where(rel == OWN, (idxv & (V - 1)) - V, 0).reshape(N)
            cp_row.start()
            first_v[...] = first.reshape(N)
            cp_first.start()

            ms = [(rel == o).astype(jnp.float32) for o in range(N_DEV)]
            m = jnp.concatenate(ms, axis=0).astype(jnp.bfloat16)
            ra = lax.broadcasted_iota(jnp.int32, (128, 256), 0)
            rb = lax.broadcasted_iota(jnp.int32, (128, 256), 1)
            rhs = jnp.where((ra < rb), 1.0, 0.0).astype(jnp.bfloat16)
            ee = jnp.dot(m, rhs, preferred_element_type=jnp.float32)
            e = ee[:, :128]
            tot = ee[:, 128:]
            li = lax.broadcasted_iota(jnp.int32, (64, 64), 0)
            lj = lax.broadcasted_iota(jnp.int32, (64, 64), 1)
            lm = jnp.where(((li >> 4) == (lj >> 4)) & (lj < li), 1.0, 0.0).astype(jnp.bfloat16)
            off = jnp.dot(lm, tot.astype(jnp.bfloat16), preferred_element_type=jnp.float32)
            rk = e + off
            slot = ms[0] * rk[0:16]
            for o in range(1, N_DEV):
                slot = slot + ms[o] * (rk[16 * o:16 * o + 16] + float(o * N))
            inc = off + tot
            slot_v[...] = (slot.astype(jnp.int32) * 4).reshape(N)
            cp_slot.start()
            meta_v[0:16, :] = ((rk[16 * DIAG:16 * DIAG + 16] + ms[DIAG]).astype(jnp.int32) + (C - 1)) >> LC
            tl = jnp.zeros((8, 128), jnp.float32)
            for o in range(N_DEV):
                tl = jnp.where(sub == o, jnp.broadcast_to(inc[16 * o + 15:16 * o + 16], (8, 128)), tl)
            meta_v[16:24, :] = jnp.maximum((tl.astype(jnp.int32) + 1) & -2, 2)
            cp_meta.start()

        def step(raw, t, carry):
            cnt, issued, sent = carry
            if raw:
                @pl.when(t == I0 // S)
                def _():
                    cp_s1.wait()

                @pl.when(t == TB)
                def _():
                    with scope("vec"):
                        vector_phase()
            for i in range(S):
                if raw:
                    v = ((idx_s[t * S + i] - base) & (N_DEV * V - 1)) - V
                else:
                    v = row_s[t * S + i]
                lst[cnt] = v
                cnt = cnt + lax.shift_right_logical(v, 31)
            new_issued = cnt >> LC
            loop(issued, new_issued, issue_gather)
            if raw:
                lag = jnp.where(t < TL, LAG, jnp.where(t == TB - 1, LAGB, LAG2))
            else:
                lag = LAG2
            new_sent = jnp.maximum(sent, new_issued - lag)
            loop(sent, new_sent, pack_send)
            return cnt, new_issued, new_sent

        with scope("phA"):
            carry = lax.fori_loop(0, P0 // S, functools.partial(step, True), (jnp.int32(0),) * 3)
        with scope("roww"):
            cp_row.wait()
        with scope("phA2"):
            cnt, issued, sent = lax.fori_loop(P0 // S, N // S, functools.partial(step, False), carry)
        for i in range(C):
            lst[cnt + i] = 0
        c_me = jnp.maximum((cnt + 1) & -2, 2)
        n_me = (c_me + C - 1) >> LC
        loop(issued, n_me, issue_gather)

        k_me = n_me - 1
        r_me = c_me - (k_me << LC)
        loop(sent, k_me, pack_send)
        pack(k_me)

        @pl.when((k_me <= K0) & is_mid)
        def _():
            catch_up(k_me)

        def send_last(sz):
            send_l(k_me, sz)
            send_r(k_me, sz)
        sized(r_me, send_last)

        cp_first.wait()
        cp_slot.wait()
        cp_meta.wait()

        c_l, c_r, c_d = meta_s[16 + FROM_L, 0], meta_s[16 + FROM_R, 0], meta_s[16 + DIAG, 0]
        k_l, k_r, k_d = (c_l - 1) >> LC, (c_r - 1) >> LC, (c_d - 1) >> LC
        r_l, r_r, r_d = c_l - (k_l << LC), c_r - (k_r << LC), c_d - (k_d << LC)
        n_l, n_d = k_l + 1, k_d + 1
        d1 = (c_d - c_me) >> LC
        d2 = (c_me - c_d) >> LC

        def via_left(k, d):
            return (k < d) | ((k >= jnp.abs(d)) & (((k + d) & 1) == 0))

        def fwd_l(k, sz=C):
            rcopy(FROM_L, DIAG, k, right, n_me + k, sz).start()

        def fwd_r(k, sz=C):
            rcopy(FROM_R, DIAG, k, left, n_d + k, sz).start()

        def fwd(k, nf):
            f1 = (k < k_l) & via_left(k, d1)
            f2 = (k < k_r) & jnp.logical_not(via_left(k, d2))

            @pl.when(k < k_l)
            def _():
                wait_recv(FROM_L, k, k)

            @pl.when(f1)
            def _():
                fwd_l(k)

            @pl.when(k < k_r)
            def _():
                wait_recv(FROM_R, k, M - 1 - k)

            @pl.when(f2)
            def _():
                fwd_r(k)
            return nf + f1.astype(jnp.int32) + f2.astype(jnp.int32)

        with scope("phC"):
            n_f = lax.fori_loop(0, jnp.maximum(k_l, k_r), fwd, jnp.int32(0))

            def last_l(sz):
                wait_recv(FROM_L, k_l, k_l, sz)

                @pl.when(via_left(k_l, d1))
                def _():
                    fwd_l(k_l, sz)

            def last_r(sz):
                wait_recv(FROM_R, k_r, M - 1 - k_r, sz)

                @pl.when(jnp.logical_not(via_left(k_r, d2)))
                def _():
                    fwd_r(k_r, sz)
            sized(r_l, last_l)
            sized(r_r, last_r)
        n_s = n_f + 2 * k_me

        def ws2(sz):
            wait_send(sz=sz)
            wait_send(sz=sz)
        sized(r_me, ws2)

        @pl.when(via_left(k_l, d1))
        def _():
            sized(r_l, lambda sz: wait_send(sz=sz))

        @pl.when(jnp.logical_not(via_left(k_r, d2)))
        def _():
            sized(r_r, lambda sz: wait_send(sz=sz))

        def wait_diag(have, need):
            loop(have, jnp.minimum(need, k_d), lambda k: wait_recv(DIAG, k, n_l + k))

            @pl.when((need == n_d) & (have < n_d))
            def _():
                sized(r_d, lambda sz: wait_recv(DIAG, k_d, n_l + k_d, sz))

        def blk(b, carry):
            have, done = carry
            for g in range(128 // G):
                c0 = g * G
                need = meta_s[b, c0 + G - 1]
                wait_diag(have, need)
                have = need
                p0 = pl.multiple_of(b * 128 + c0, G)
                rows = [pbuf[pl.ds(pl.multiple_of(slot_s[first_s[p0 + r]], 4), 4), :] for r in range(G)]
                w = jnp.concatenate(
                    [jnp.concatenate([x[j:j + 1, :] for x in rows], axis=0) for j in range(4)], axis=1)
                hi = pltpu.bitcast(w & jnp.uint32(0xFFFF0000), jnp.float32)
                lo = pltpu.bitcast(w << 16, jnp.float32)
                out_ref[pl.ds(p0, G), 0:H] = hi.astype(out_ref.dtype)
                out_ref[pl.ds(p0, G), H:D] = lo.astype(out_ref.dtype)
                if g == 0:
                    tgt = n_s - ((n_f * (NB - b + FLAG)) >> 4)
                    loop(done, tgt, wait_send)
                    done = jnp.maximum(tgt, done)
            return have, done

        with scope("phD"):
            have, done = lax.fori_loop(0, NB, blk, (jnp.int32(0), jnp.int32(0)))
        wait_diag(have, n_d)
        with scope("fin"):
            loop(done, n_s, wait_send)

    return pl.pallas_call(
        body,
        out_shape=jax.ShapeDtypeStruct((N, D), jnp.bfloat16),
        in_specs=[pl.BlockSpec(memory_space=pl.ANY)] * 3,
        out_specs=pl.BlockSpec(memory_space=pltpu.VMEM),
        scratch_shapes=[
            pltpu.SMEM((P0,), jnp.int32),
            pltpu.SMEM((N + C,), jnp.int32),
            pltpu.SMEM((N,), jnp.int32),
            pltpu.SMEM((N,), jnp.int32),
            pltpu.SMEM((N,), jnp.int32),
            pltpu.SMEM((24, 128), jnp.int32),
            pltpu.VMEM((NB, 128), jnp.int32),
            pltpu.VMEM((N,), jnp.int32),
            pltpu.VMEM((N,), jnp.int32),
            pltpu.VMEM((N,), jnp.int32),
            pltpu.VMEM((24, 128), jnp.int32),
            pltpu.VMEM((NCH, C, D), jnp.float32),
            pltpu.VMEM((N_DEV * N * 4, 128), jnp.uint32),
            pltpu.SemaphoreType.DMA((7,)),
            pltpu.SemaphoreType.DMA((NG,)),
            pltpu.SemaphoreType.DMA,
            pltpu.SemaphoreType.DMA((M,)),
            pltpu.SemaphoreType.REGULAR,
        ],
        compiler_params=pltpu.CompilerParams(
            collective_id=0, vmem_limit_bytes=64 << 20,
            disable_bounds_checks=True, disable_semaphore_checks=True),
    )(idx, idx2, table)
```

```python
import functools

import jax
import jax.numpy as jnp
from jax import lax
from jax.experimental import pallas as pl
from jax.experimental.pallas import tpu as pltpu

N_DEV = 4
N = 2048
V = 16384
LV = 14
D = 1024
H = D // 2
LC = 3
C = 1 << LC
NCH = N // C
M = NCH + 3
NB = N // 128
S = 32
LAG = 2
NG = 16
G = 32
I0 = 128
K0 = 2
TB = 16
PB0 = 5
P0 = 128 * PB0
MESH = pl.DeviceIdType.MESH
OWN, FROM_R, DIAG, FROM_L = 0, 1, 2, 3


def pallas_dist_embed_lookup_i_n2048_v16384_d1024_kernel(table, idx):
    idx = idx.astype(jnp.int32)
    idx2 = idx.reshape(NB, 128)

    def body(idx_hbm, idx2_hbm, tab_ref, out_ref,
             idx_s, lst, row_s, first_s, slot_s, meta_s,
             idx_v, row_v, first_v, slot_v, meta_v, gbuf, pbuf,
             misc_sem, gsem, ssem, rsem, rdy):
        me = lax.axis_index("i")
        left = (me + 3) & 3
        right = (me + 1) & 3
        is_mid = (me & 1) == 1

        cp_s0 = pltpu.make_async_copy(
            idx_hbm.at[pl.ds(0, I0)], idx_s.at[pl.ds(0, I0)], misc_sem.at[0])
        cp_s0.start()

        bar = pltpu.get_barrier_semaphore()

        @pl.when(me != 2)
        def _():
            for nb in (left, right):
                pl.semaphore_signal(bar, inc=1, device_id=(nb,), device_id_type=MESH)

        cp_s1 = pltpu.make_async_copy(
            idx_hbm.at[pl.ds(I0, P0 - I0)], idx_s.at[pl.ds(I0, P0 - I0)], misc_sem.at[1])
        cp_s1.start()
        cp_v = pltpu.make_async_copy(idx2_hbm, idx_v, misc_sem.at[2])
        cp_v.start()
        cp_row = pltpu.make_async_copy(row_v, row_s, misc_sem.at[3])
        cp_first = pltpu.make_async_copy(first_v, first_s, misc_sem.at[4])
        cp_slot = pltpu.make_async_copy(slot_v, slot_s, misc_sem.at[5])
        cp_meta = pltpu.make_async_copy(meta_v, meta_s, misc_sem.at[6])

        @pl.when(me == 2)
        def _():
            pl.semaphore_wait(bar, 2)
            for nb in (left, right):
                pl.semaphore_signal(rdy, inc=1, device_id=(nb,), device_id_type=MESH)

        cp_s0.wait()

        def chunk_start(reg, k):
            return pl.multiple_of((reg * N + k * C) * 4, 4 * C)

        def rcopy(src_reg, dst_reg, k, tgt, si, sz=C):
            return pltpu.make_async_remote_copy(
                src_ref=pbuf.at[pl.ds(chunk_start(src_reg, k), 4 * sz)],
                dst_ref=pbuf.at[pl.ds(chunk_start(dst_reg, k), 4 * sz)],
                send_sem=ssem, recv_sem=rsem.at[si],
                device_id=(tgt,), device_id_type=MESH)

        def wait_recv(reg, k, si, sz=C):
            rcopy(reg, reg, k, me, si, sz).wait_recv()

        def wait_send(_=None, sz=C):
            rcopy(OWN, OWN, 0, me, 0, sz).wait_send()

        def sized(r, fn):
            lax.switch((r >> 1) - 1,
                       [functools.partial(fn, s) for s in range(2, C + 1, 2)])

        def loop(lo, hi, fn):
            def b(k, c):
                fn(k)
                return c
            lax.fori_loop(lo, hi, b, 0)

        def send_l(k, sz=C):
            rcopy(OWN, FROM_R, k, left, M - 1 - k, sz).start()

        def send_r(k, sz=C):
            rcopy(OWN, FROM_L, k, right, k, sz).start()

        def catch_up(n):
            pl.semaphore_wait(rdy, 1)

            @pl.when(me == 3)
            def _():
                loop(0, n, send_l)

            @pl.when(me == 1)
            def _():
                loop(0, n, send_r)

        def issue_gather(k):
            for r in range(C):
                row = lst[k * C + r] & (V - 1)
                pltpu.make_async_copy(
                    tab_ref.at[pl.ds(row, 1)],
                    gbuf.at[k, pl.ds(r, 1)], gsem.at[k & (NG - 1)]).start()

        def pack(k):
            pltpu.make_async_copy(gbuf.at[k], gbuf.at[k], gsem.at[k & (NG - 1)]).wait()
            xb = pltpu.bitcast(
                gbuf[k].astype(jnp.bfloat16).astype(jnp.float32), jnp.uint32)
            w = xb[:, :H] | (xb[:, H:] >> 16)
            pbuf[pl.ds(chunk_start(OWN, k), 4 * C), :] = w.reshape(4 * C, 128)

            @pl.when(k == 0)
            def _():
                @pl.when(me == 0)
                def _():
                    pl.semaphore_wait(bar, 2)

                @pl.when(is_mid)
                def _():
                    pl.semaphore_wait(bar, 1)

        def pack_send(k):
            pack(k)

            @pl.when((k == K0) & is_mid)
            def _():
                catch_up(K0)

            @pl.when((k >= K0) | (me != 3))
            def _():
                send_l(k)

            @pl.when((k >= K0) | (me != 1))
            def _():
                send_r(k)

        def find_repeats():
            cp_v.wait()
            idxv = idx_v[...] & (N_DEV * V - 1)
            pos = (lax.broadcasted_iota(jnp.int32, (NB, 128), 0) * 128
                   + lax.broadcasted_iota(jnp.int32, (NB, 128), 1))
            sub = lax.broadcasted_iota(jnp.int32, (8, 128), 0)
            idx_t = idxv.T
            rows = {pb: jnp.broadcast_to(idxv[pb:pb + 1, :], (8, 128))
                    for pb in range(PB0, NB)}
            acc = {pb: jnp.full((8, 128), N, jnp.int32) for pb in range(PB0, NB)}
            for b in range(NB - 1, -1, -1):
                xb = jnp.broadcast_to(idx_t[:, b:b + 1], (128, 128))
                for u in range(15, -1, -1):
                    xq = xb[8 * u:8 * u + 8]
                    qv = sub + (128 * b + 8 * u)
                    for pb in range(max(b, PB0), NB):
                        acc[pb] = jnp.where(xq == rows[pb], qv, acc[pb])
            first = jnp.concatenate(
                [pos[0:PB0]]
                + [jnp.min(acc[pb], axis=0, keepdims=True) for pb in range(PB0, NB)],
                axis=0)
            rel = jnp.where(first == pos, ((idxv >> LV) - me) & 3, N_DEV)
            row_v[...] = jnp.where(rel == OWN, (idxv & (V - 1)) - V, 0).reshape(N)
            cp_row.start()
            first_v[...] = first.reshape(N)
            cp_first.start()
            idx_v[...] = rel

        def find_slots():
            rel = idx_v[...]
            sub = lax.broadcasted_iota(jnp.int32, (8, 128), 0)
            ms = [(rel == o).astype(jnp.float32) for o in range(N_DEV)]
            m = jnp.concatenate(ms, axis=0).astype(jnp.bfloat16)
            ra = lax.broadcasted_iota(jnp.int32, (128, 256), 0)
            rb = lax.broadcasted_iota(jnp.int32, (128, 256), 1)
            rhs = jnp.where(ra < rb, 1.0, 0.0).astype(jnp.bfloat16)
            ee = jnp.dot(m, rhs, preferred_element_type=jnp.float32)
            tot = ee[:, 128:]
            li = lax.broadcasted_iota(jnp.int32, (64, 64), 0)
            lj = lax.broadcasted_iota(jnp.int32, (64, 64), 1)
            lm = jnp.where(((li >> 4) == (lj >> 4)) & (lj < li), 1.0, 0.0)
            off = jnp.dot(lm.astype(jnp.bfloat16), tot.astype(jnp.bfloat16),
                          preferred_element_type=jnp.float32)
            rk = ee[:, :128] + off
            slot = ms[0] * rk[0:NB]
            for o in range(1, N_DEV):
                slot = slot + ms[o] * (rk[NB * o:NB * o + NB] + float(o * N))
            slot_v[...] = (slot.astype(jnp.int32) * 4).reshape(N)
            cp_slot.start()
            meta_v[0:NB, :] = jnp.maximum((
                (rk[NB * DIAG:NB * DIAG + NB] + ms[DIAG]).astype(jnp.int32) + (C - 1)
            ) >> LC, 1)
            inc = off + tot
            tl = jnp.zeros((8, 128), jnp.float32)
            for o in range(N_DEV):
                last = inc[NB * o + NB - 1:NB * o + NB]
                tl = jnp.where(sub == o, jnp.broadcast_to(last, (8, 128)), tl)
            meta_v[NB:NB + 8, :] = jnp.maximum((tl.astype(jnp.int32) + 1) & -2, 2)
            cp_meta.start()

        base = me * V

        def step(raw, t, carry):
            cnt, issued, sent = carry
            if raw:
                @pl.when(t == I0 // S)
                def _():
                    cp_s1.wait()

                @pl.when(t == TB)
                def _():
                    find_repeats()
            for i in range(S):
                if raw:
                    v = ((idx_s[t * S + i] - base) & (N_DEV * V - 1)) - V
                else:
                    v = row_s[t * S + i]
                lst[cnt] = v
                cnt = cnt + lax.shift_right_logical(v, 31)
            new_issued = cnt >> LC
            loop(issued, new_issued, issue_gather)
            lag = jnp.where(t == TB - 1, 1, LAG) if raw else LAG
            new_sent = jnp.maximum(sent, new_issued - lag)
            loop(sent, new_sent, pack_send)
            return cnt, new_issued, new_sent

        carry = lax.fori_loop(0, P0 // S, functools.partial(step, True),
                              (jnp.int32(0),) * 3)
        cp_row.wait()
        cnt, issued, sent = lax.fori_loop(
            P0 // S, N // S, functools.partial(step, False), carry)
        for i in range(C):
            lst[cnt + i] = 0
        c_me = jnp.maximum((cnt + 1) & -2, 2)
        n_me = (c_me + C - 1) >> LC
        loop(issued, n_me, issue_gather)
        find_slots()

        k_me = n_me - 1
        r_me = c_me - (k_me << LC)
        loop(sent, k_me, pack_send)
        pack(k_me)

        @pl.when((k_me <= K0) & is_mid)
        def _():
            catch_up(k_me)

        def send_last(sz):
            send_l(k_me, sz)
            send_r(k_me, sz)
        sized(r_me, send_last)

        cp_first.wait()
        cp_slot.wait()
        cp_meta.wait()

        c_l, c_r, c_d = meta_s[NB + FROM_L, 0], meta_s[NB + FROM_R, 0], meta_s[NB + DIAG, 0]
        k_l, k_r, k_d = (c_l - 1) >> LC, (c_r - 1) >> LC, (c_d - 1) >> LC
        r_l, r_r, r_d = c_l - (k_l << LC), c_r - (k_r << LC), c_d - (k_d << LC)
        n_l, n_d = k_l + 1, k_d + 1

        def via_left(k, d):
            return (k < d) | ((k >= jnp.abs(d)) & (((k + d) & 1) == 0))

        d1 = (c_d - c_me) >> LC
        d2 = (c_me - c_d) >> LC
        fwd_last_l = via_left(k_l, d1)
        fwd_last_r = jnp.logical_not(via_left(k_r, d2))

        def fwd_l(k, sz=C):
            rcopy(FROM_L, DIAG, k, right, n_me + k, sz).start()

        def fwd_r(k, sz=C):
            rcopy(FROM_R, DIAG, k, left, n_d + k, sz).start()

        def fwd(k, nf):
            f1 = (k < k_l) & via_left(k, d1)
            f2 = (k < k_r) & jnp.logical_not(via_left(k, d2))

            @pl.when(k < k_l)
            def _():
                wait_recv(FROM_L, k, k)

            @pl.when(f1)
            def _():
                fwd_l(k)

            @pl.when(k < k_r)
            def _():
                wait_recv(FROM_R, k, M - 1 - k)

            @pl.when(f2)
            def _():
                fwd_r(k)
            return nf + f1.astype(jnp.int32) + f2.astype(jnp.int32)

        n_f = lax.fori_loop(0, jnp.maximum(k_l, k_r), fwd, jnp.int32(0))

        def last_l(sz):
            wait_recv(FROM_L, k_l, k_l, sz)

            @pl.when(fwd_last_l)
            def _():
                fwd_l(k_l, sz)

        def last_r(sz):
            wait_recv(FROM_R, k_r, M - 1 - k_r, sz)

            @pl.when(fwd_last_r)
            def _():
                fwd_r(k_r, sz)

        sized(r_l, last_l)
        sized(r_r, last_r)

        n_s = n_f + 2 * k_me

        def wait_send2(sz):
            wait_send(sz=sz)
            wait_send(sz=sz)
        sized(r_me, wait_send2)

        @pl.when(fwd_last_l)
        def _():
            sized(r_l, lambda sz: wait_send(sz=sz))

        @pl.when(fwd_last_r)
        def _():
            sized(r_r, lambda sz: wait_send(sz=sz))

        def wait_diag(have, need):
            loop(have, jnp.minimum(need, k_d), lambda k: wait_recv(DIAG, k, n_l + k))

            @pl.when((need == n_d) & (have < n_d))
            def _():
                sized(r_d, lambda sz: wait_recv(DIAG, k_d, n_l + k_d, sz))

        def blk(b, carry):
            have, done = carry
            for g in range(128 // G):
                c0 = g * G
                need = meta_s[b, c0 + G - 1]
                wait_diag(have, need)
                have = need
                p0 = pl.multiple_of(b * 128 + c0, G)
                rows = [pbuf[pl.ds(pl.multiple_of(slot_s[first_s[p0 + r]], 4), 4), :]
                        for r in range(G)]
                w = jnp.concatenate(
                    [jnp.concatenate([x[j:j + 1, :] for x in rows], axis=0)
                     for j in range(4)], axis=1)
                hi = pltpu.bitcast(w & jnp.uint32(0xFFFF0000), jnp.float32)
                lo = pltpu.bitcast(w << 16, jnp.float32)
                out_ref[pl.ds(p0, G), 0:H] = hi.astype(out_ref.dtype)
                out_ref[pl.ds(p0, G), H:D] = lo.astype(out_ref.dtype)
                if g == 1:
                    tgt = n_s - ((n_f * (NB - 1 - b)) >> 3)
                    loop(done, tgt, wait_send)
                    done = jnp.maximum(tgt, done)
            return have, done

        lax.fori_loop(0, NB, blk, (jnp.int32(0), jnp.int32(0)))

    return pl.pallas_call(
        body,
        out_shape=jax.ShapeDtypeStruct((N, D), jnp.bfloat16),
        in_specs=[pl.BlockSpec(memory_space=pl.ANY)] * 3,
        out_specs=pl.BlockSpec(memory_space=pltpu.VMEM),
        scratch_shapes=[
            pltpu.SMEM((P0,), jnp.int32),
            pltpu.SMEM((N + C,), jnp.int32),
            pltpu.SMEM((N,), jnp.int32),
            pltpu.SMEM((N,), jnp.int32),
            pltpu.SMEM((N,), jnp.int32),
            pltpu.SMEM((NB + 8, 128), jnp.int32),
            pltpu.VMEM((NB, 128), jnp.int32),
            pltpu.VMEM((N,), jnp.int32),
            pltpu.VMEM((N,), jnp.int32),
            pltpu.VMEM((N,), jnp.int32),
            pltpu.VMEM((NB + 8, 128), jnp.int32),
            pltpu.VMEM((NCH, C, D), jnp.float32),
            pltpu.VMEM((N_DEV * N * 4, 128), jnp.uint32),
            pltpu.SemaphoreType.DMA((7,)),
            pltpu.SemaphoreType.DMA((NG,)),
            pltpu.SemaphoreType.DMA,
            pltpu.SemaphoreType.DMA((M,)),
            pltpu.SemaphoreType.REGULAR,
        ],
        compiler_params=pltpu.CompilerParams(
            collective_id=0, vmem_limit_bytes=64 << 20,
            disable_bounds_checks=True, disable_semaphore_checks=True),
    )(idx, idx2, table)
```

```python
import functools

import jax
import jax.numpy as jnp
from jax import lax
from jax.experimental import pallas as pl
from jax.experimental.pallas import tpu as pltpu

N_DEV = 4
N = 2048
V = 16384
LV = 14
D = 1024
H = D // 2
LC = 3
C = 1 << LC
NCH = N // C
M = NCH + 3
NB = N // 128
S = 32
NG = 16
G = 32
I0 = 128
K0 = 2
KEEP = 2
HEAD = 16
TB = 16
PB0 = 5
P0 = 128 * PB0
MESH = pl.DeviceIdType.MESH
OWN, FROM_R, DIAG, FROM_L = 0, 1, 2, 3


def pallas_dist_embed_lookup_i_n2048_v16384_d1024_kernel(table, idx):
    idx = idx.astype(jnp.int32)
    idx2 = idx.reshape(NB, 128)

    def body(idx_hbm, idx2_hbm, tab_ref, out_ref,
             idx_s, lst, row_s, first_s, slot_s, meta_s,
             idx_v, row_v, first_v, slot_v, meta_v, gbuf, pbuf,
             misc_sem, gsem, ssem, rsem, rdy):
        me = lax.axis_index("i")
        left = (me + 3) & 3
        right = (me + 1) & 3
        is_mid = (me & 1) == 1

        cp_s0 = pltpu.make_async_copy(
            idx_hbm.at[pl.ds(0, I0)], idx_s.at[pl.ds(0, I0)], misc_sem.at[0])
        cp_s0.start()

        bar = pltpu.get_barrier_semaphore()

        @pl.when(me != 2)
        def _():
            for nb in (left, right):
                pl.semaphore_signal(bar, inc=1, device_id=(nb,), device_id_type=MESH)

        cp_s1 = pltpu.make_async_copy(
            idx_hbm.at[pl.ds(I0, P0 - I0)], idx_s.at[pl.ds(I0, P0 - I0)], misc_sem.at[1])
        cp_s1.start()
        cp_v = pltpu.make_async_copy(idx2_hbm, idx_v, misc_sem.at[2])
        cp_v.start()
        cp_row = pltpu.make_async_copy(row_v, row_s, misc_sem.at[3])
        cp_first = pltpu.make_async_copy(first_v, first_s, misc_sem.at[4])
        cp_slot = pltpu.make_async_copy(slot_v, slot_s, misc_sem.at[5])
        cp_meta = pltpu.make_async_copy(meta_v, meta_s, misc_sem.at[6])

        @pl.when(me == 2)
        def _():
            pl.semaphore_wait(bar, 2)
            for nb in (left, right):
                pl.semaphore_signal(rdy, inc=1, device_id=(nb,), device_id_type=MESH)

        cp_s0.wait()

        def chunk_start(reg, k):
            return pl.multiple_of((reg * N + k * C) * 4, 4 * C)

        def rcopy(src_reg, dst_reg, k, tgt, si, sz=C):
            return pltpu.make_async_remote_copy(
                src_ref=pbuf.at[pl.ds(chunk_start(src_reg, k), 4 * sz)],
                dst_ref=pbuf.at[pl.ds(chunk_start(dst_reg, k), 4 * sz)],
                send_sem=ssem, recv_sem=rsem.at[si],
                device_id=(tgt,), device_id_type=MESH)

        def wait_recv(reg, k, si, sz=C):
            rcopy(reg, reg, k, me, si, sz).wait_recv()

        def wait_send(_=None, sz=C):
            rcopy(OWN, OWN, 0, me, 0, sz).wait_send()

        def sized(r, fn):
            lax.switch((r >> 1) - 1,
                       [functools.partial(fn, s) for s in range(2, C + 1, 2)])

        def loop(lo, hi, fn):
            def b(k, c):
                fn(k)
                return c
            lax.fori_loop(lo, hi, b, 0)

        def send_l(k, sz=C):
            rcopy(OWN, FROM_R, k, left, M - 1 - k, sz).start()

        def send_r(k, sz=C):
            rcopy(OWN, FROM_L, k, right, k, sz).start()

        def catch_up(n):
            pl.semaphore_wait(rdy, 1)

            @pl.when(me == 3)
            def _():
                loop(0, n, send_l)

            @pl.when(me == 1)
            def _():
                loop(0, n, send_r)

        def issue_gather(k):
            for r in range(C):
                row = lst[k * C + r] & (V - 1)
                pltpu.make_async_copy(
                    tab_ref.at[pl.ds(row, 1)],
                    gbuf.at[k, pl.ds(r, 1)], gsem.at[k & (NG - 1)]).start()

        def pack(k):
            pltpu.make_async_copy(gbuf.at[k], gbuf.at[k], gsem.at[k & (NG - 1)]).wait()
            xb = pltpu.bitcast(
                gbuf[k].astype(jnp.bfloat16).astype(jnp.float32), jnp.uint32)
            w = xb[:, :H] | (xb[:, H:] >> 16)
            pbuf[pl.ds(chunk_start(OWN, k), 4 * C), :] = w.reshape(4 * C, 128)

            @pl.when(k == 0)
            def _():
                @pl.when(me == 0)
                def _():
                    pl.semaphore_wait(bar, 2)

                @pl.when(is_mid)
                def _():
                    pl.semaphore_wait(bar, 1)

        def pack_send(k):
            pack(k)

            @pl.when((k == K0) & is_mid)
            def _():
                catch_up(K0)

            @pl.when((k >= K0) | (me != 3))
            def _():
                send_l(k)

            @pl.when((k >= K0) | (me != 1))
            def _():
                send_r(k)

        def find_repeats():
            cp_v.wait()
            idxv = idx_v[...] & (N_DEV * V - 1)
            pos = (lax.broadcasted_iota(jnp.int32, (NB, 128), 0) * 128
                   + lax.broadcasted_iota(jnp.int32, (NB, 128), 1))
            sub = lax.broadcasted_iota(jnp.int32, (8, 128), 0)
            idx_t = idxv.T
            rows = {pb: jnp.broadcast_to(idxv[pb:pb + 1, :], (8, 128))
                    for pb in range(PB0, NB)}
            acc = {pb: jnp.full((8, 128), N, jnp.int32) for pb in range(PB0, NB)}
            for b in range(NB - 1, -1, -1):
                xb = jnp.broadcast_to(idx_t[:, b:b + 1], (128, 128))
                for u in range(15, -1, -1):
                    xq = xb[8 * u:8 * u + 8]
                    qv = sub + (128 * b + 8 * u)
                    for pb in range(max(b, PB0), NB):
                        acc[pb] = lax.select(lax.eq(xq, rows[pb]), qv, acc[pb])
            first = jnp.concatenate(
                [pos[0:PB0]]
                + [jnp.min(acc[pb], axis=0, keepdims=True) for pb in range(PB0, NB)],
                axis=0)
            rel = jnp.where(first == pos, ((idxv >> LV) - me) & 3, N_DEV)
            row_v[...] = jnp.where(rel == OWN, (idxv & (V - 1)) - V, 0).reshape(N)
            cp_row.start()
            first_v[...] = first.reshape(N)
            cp_first.start()
            idx_v[...] = rel

        def find_slots():
            rel = idx_v[...]
            sub = lax.broadcasted_iota(jnp.int32, (8, 128), 0)
            ms = [(rel == o).astype(jnp.float32) for o in range(N_DEV)]
            m = jnp.concatenate(ms, axis=0).astype(jnp.bfloat16)
            ra = lax.broadcasted_iota(jnp.int32, (128, 256), 0)
            rb = lax.broadcasted_iota(jnp.int32, (128, 256), 1)
            rhs = jnp.where(ra < rb, 1.0, 0.0).astype(jnp.bfloat16)
            ee = jnp.dot(m, rhs, preferred_element_type=jnp.float32)
            tot = ee[:, 128:]
            li = lax.broadcasted_iota(jnp.int32, (64, 64), 0)
            lj = lax.broadcasted_iota(jnp.int32, (64, 64), 1)
            lm = jnp.where(((li >> 4) == (lj >> 4)) & (lj < li), 1.0, 0.0)
            off = jnp.dot(lm.astype(jnp.bfloat16), tot.astype(jnp.bfloat16),
                          preferred_element_type=jnp.float32)
            rk = ee[:, :128] + off
            slot = ms[0] * rk[0:NB]
            for o in range(1, N_DEV):
                slot = slot + ms[o] * (rk[NB * o:NB * o + NB] + float(o * N))
            slot_v[...] = (slot.astype(jnp.int32) * 4).reshape(N)
            cp_slot.start()
            meta_v[0:NB, :] = jnp.maximum((
                (rk[NB * DIAG:NB * DIAG + NB] + ms[DIAG]).astype(jnp.int32) + (C - 1)
            ) >> LC, 1)
            inc = off + tot
            tl = jnp.zeros((8, 128), jnp.float32)
            for o in range(N_DEV):
                last = inc[NB * o + NB - 1:NB * o + NB]
                tl = jnp.where(sub == o, jnp.broadcast_to(last, (8, 128)), tl)
            meta_v[NB:NB + 8, :] = jnp.maximum((tl.astype(jnp.int32) + 1) & -2, 2)
            cp_meta.start()

        base = me * V

        def step(raw, t, carry):
            cnt, issued, before, sent = carry
            if raw:
                @pl.when(t == I0 // S)
                def _():
                    cp_s1.wait()

                @pl.when(t == TB)
                def _():
                    find_repeats()
            for i in range(S):
                if raw:
                    v = ((idx_s[t * S + i] - base) & (N_DEV * V - 1)) - V
                else:
                    v = row_s[t * S + i]
                lst[cnt] = v
                cnt = cnt + lax.shift_right_logical(v, 31)
            new_issued = cnt >> LC
            loop(issued, new_issued, issue_gather)
            ready = jnp.where(t == TB - 1, issued, before) if raw else before
            new_sent = jnp.maximum(sent, jnp.minimum(ready, new_issued - 1))
            loop(sent, new_sent, pack_send)
            return cnt, new_issued, issued, new_sent

        carry = lax.fori_loop(0, P0 // S, functools.partial(step, True),
                              (jnp.int32(0),) * 4)
        cp_row.wait()
        cnt, issued, _, sent = lax.fori_loop(
            P0 // S, N // S, functools.partial(step, False), carry)
        for i in range(C):
            lst[cnt + i] = 0
        c_me = jnp.maximum((cnt + 1) & -2, 2)
        n_me = (c_me + C - 1) >> LC
        loop(issued, n_me, issue_gather)
        find_slots()

        k_me = n_me - 1
        r_me = c_me - (k_me << LC)
        loop(sent, k_me, pack_send)
        pack(k_me)

        @pl.when((k_me <= K0) & is_mid)
        def _():
            catch_up(k_me)

        def send_last(sz):
            send_l(k_me, sz)
            send_r(k_me, sz)
        sized(r_me, send_last)

        cp_first.wait()
        cp_slot.wait()
        cp_meta.wait()

        c_l, c_r, c_d = meta_s[NB + FROM_L, 0], meta_s[NB + FROM_R, 0], meta_s[NB + DIAG, 0]
        k_l, k_r, k_d = (c_l - 1) >> LC, (c_r - 1) >> LC, (c_d - 1) >> LC
        r_l, r_r, r_d = c_l - (k_l << LC), c_r - (k_r << LC), c_d - (k_d << LC)
        n_l, n_d = k_l + 1, k_d + 1

        def via_left(k, d):
            return (k < d) | ((k >= jnp.abs(d)) & (((k + d) & 1) == 0))

        x = c_me - c_d + jnp.where(me == 0, -HEAD, jnp.where(me == 2, HEAD, 0))
        d1 = (-x) >> LC
        d2 = x >> LC
        fwd_last_l = via_left(k_l, d1)
        fwd_last_r = jnp.logical_not(via_left(k_r, d2))

        def fwd_l(k, sz=C):
            rcopy(FROM_L, DIAG, k, right, n_me + k, sz).start()

        def fwd_r(k, sz=C):
            rcopy(FROM_R, DIAG, k, left, n_d + k, sz).start()

        def fwd(k, nf):
            f1 = (k < k_l) & via_left(k, d1)
            f2 = (k < k_r) & jnp.logical_not(via_left(k, d2))

            @pl.when(k < k_l)
            def _():
                wait_recv(FROM_L, k, k)

            @pl.when(f1)
            def _():
                fwd_l(k)

            @pl.when(k < k_r)
            def _():
                wait_recv(FROM_R, k, M - 1 - k)

            @pl.when(f2)
            def _():
                fwd_r(k)
            return nf + f1.astype(jnp.int32) + f2.astype(jnp.int32)

        n_f = lax.fori_loop(0, jnp.maximum(k_l, k_r), fwd, jnp.int32(0))

        def last_l(sz):
            wait_recv(FROM_L, k_l, k_l, sz)

            @pl.when(fwd_last_l)
            def _():
                fwd_l(k_l, sz)

        def last_r(sz):
            wait_recv(FROM_R, k_r, M - 1 - k_r, sz)

            @pl.when(fwd_last_r)
            def _():
                fwd_r(k_r, sz)

        sized(r_l, last_l)
        sized(r_r, last_r)

        n_s = n_f + 2 * k_me

        def wait_send2(sz):
            wait_send(sz=sz)
            wait_send(sz=sz)
        sized(r_me, wait_send2)

        @pl.when(fwd_last_l)
        def _():
            sized(r_l, lambda sz: wait_send(sz=sz))

        @pl.when(fwd_last_r)
        def _():
            sized(r_r, lambda sz: wait_send(sz=sz))

        def wait_diag(have, need):
            loop(have, jnp.minimum(need, k_d), lambda k: wait_recv(DIAG, k, n_l + k))

            @pl.when((need == n_d) & (have < n_d))
            def _():
                sized(r_d, lambda sz: wait_recv(DIAG, k_d, n_l + k_d, sz))

        def blk(b, carry):
            have, done = carry
            for g in range(128 // G):
                c0 = g * G
                need = meta_s[b, c0 + G - 1]
                wait_diag(have, need)
                have = need
                p0 = pl.multiple_of(b * 128 + c0, G)
                rows = [pbuf[pl.ds(pl.multiple_of(slot_s[first_s[p0 + r]], 4), 4), :]
                        for r in range(G)]
                w = jnp.concatenate(
                    [jnp.concatenate([x[j:j + 1, :] for x in rows], axis=0)
                     for j in range(4)], axis=1)
                hi = pltpu.bitcast(w & jnp.uint32(0xFFFF0000), jnp.float32)
                lo = pltpu.bitcast(w << 16, jnp.float32)
                out_ref[pl.ds(p0, G), 0:H] = hi.astype(out_ref.dtype)
                out_ref[pl.ds(p0, G), H:D] = lo.astype(out_ref.dtype)
                if g == 1:
                    tgt = n_s - KEEP - ((n_f * (NB - 1 - b)) >> 3)
                    loop(done, tgt, wait_send)
                    done = jnp.maximum(tgt, done)
            return have, done

        _, done = lax.fori_loop(0, NB, blk, (jnp.int32(0), jnp.int32(0)))
        loop(done, n_s, wait_send)

    return pl.pallas_call(
        body,
        out_shape=jax.ShapeDtypeStruct((N, D), jnp.bfloat16),
        in_specs=[pl.BlockSpec(memory_space=pl.ANY)] * 3,
        out_specs=pl.BlockSpec(memory_space=pltpu.VMEM),
        scratch_shapes=[
            pltpu.SMEM((P0,), jnp.int32),
            pltpu.SMEM((N + C,), jnp.int32),
            pltpu.SMEM((N,), jnp.int32),
            pltpu.SMEM((N,), jnp.int32),
            pltpu.SMEM((N,), jnp.int32),
            pltpu.SMEM((NB + 8, 128), jnp.int32),
            pltpu.VMEM((NB, 128), jnp.int32),
            pltpu.VMEM((N,), jnp.int32),
            pltpu.VMEM((N,), jnp.int32),
            pltpu.VMEM((N,), jnp.int32),
            pltpu.VMEM((NB + 8, 128), jnp.int32),
            pltpu.VMEM((NCH, C, D), jnp.float32),
            pltpu.VMEM((N_DEV * N * 4, 128), jnp.uint32),
            pltpu.SemaphoreType.DMA((7,)),
            pltpu.SemaphoreType.DMA((NG,)),
            pltpu.SemaphoreType.DMA,
            pltpu.SemaphoreType.DMA((M,)),
            pltpu.SemaphoreType.REGULAR,
        ],
        compiler_params=pltpu.CompilerParams(
            collective_id=0, vmem_limit_bytes=64 << 20,
            disable_bounds_checks=True, disable_semaphore_checks=True),
    )(idx, idx2, table)
```

```python
import functools

import jax
import jax.numpy as jnp
from jax import lax
from jax.experimental import pallas as pl
from jax.experimental.pallas import tpu as pltpu

N_DEV = 4
N = 2048
V = 16384
LV = 14
D = 1024
H = D // 2
LC = 3
C = 1 << LC
NCH = N // C
M = NCH + 3
NB = N // 128
S = 32
NG = 16
G = 32
I0 = 128
K0 = 2
KEEP = 2
HEAD = 16
TB = 16
PB0 = 5
P0 = 128 * PB0
MESH = pl.DeviceIdType.MESH
OWN, FROM_R, DIAG, FROM_L = 0, 1, 2, 3


def pallas_dist_embed_lookup_i_n2048_v16384_d1024_kernel(table, idx):
    idx = idx.astype(jnp.int32)
    idx2 = idx.reshape(NB, 128)

    def body(idx_hbm, idx2_hbm, tab_ref, out_ref,
             idx_s, lst, row_s, first_s, slot_s, meta_s,
             idx_v, row_v, first_v, slot_v, meta_v, gbuf, pbuf,
             misc_sem, gsem, ssem, rsem, rdy):
        me = lax.axis_index("i")
        left = (me + 3) & 3
        right = (me + 1) & 3
        is_mid = (me & 1) == 1

        cp_s0 = pltpu.make_async_copy(
            idx_hbm.at[pl.ds(0, I0)], idx_s.at[pl.ds(0, I0)], misc_sem.at[0])
        cp_s0.start()

        bar = pltpu.get_barrier_semaphore()

        @pl.when(me != 2)
        def _():
            for nb in (left, right):
                pl.semaphore_signal(bar, inc=1, device_id=(nb,), device_id_type=MESH)

        cp_s1 = pltpu.make_async_copy(
            idx_hbm.at[pl.ds(I0, P0 - I0)], idx_s.at[pl.ds(I0, P0 - I0)], misc_sem.at[1])
        cp_s1.start()
        cp_v = pltpu.make_async_copy(idx2_hbm, idx_v, misc_sem.at[2])
        cp_v.start()
        cp_row = pltpu.make_async_copy(row_v, row_s, misc_sem.at[3])
        cp_first = pltpu.make_async_copy(first_v, first_s, misc_sem.at[4])
        cp_slot = pltpu.make_async_copy(slot_v, slot_s, misc_sem.at[5])
        cp_meta = pltpu.make_async_copy(meta_v, meta_s, misc_sem.at[6])

        @pl.when(me == 2)
        def _():
            pl.semaphore_wait(bar, 2)
            for nb in (left, right):
                pl.semaphore_signal(rdy, inc=1, device_id=(nb,), device_id_type=MESH)

        cp_s0.wait()

        def chunk_start(reg, k):
            return pl.multiple_of((reg * N + k * C) * 4, 4 * C)

        def rcopy(src_reg, dst_reg, k, tgt, si, sz=C):
            return pltpu.make_async_remote_copy(
                src_ref=pbuf.at[pl.ds(chunk_start(src_reg, k), 4 * sz)],
                dst_ref=pbuf.at[pl.ds(chunk_start(dst_reg, k), 4 * sz)],
                send_sem=ssem, recv_sem=rsem.at[si],
                device_id=(tgt,), device_id_type=MESH)

        def wait_recv(reg, k, si, sz=C):
            rcopy(reg, reg, k, me, si, sz).wait_recv()

        def wait_send(_=None, sz=C):
            rcopy(OWN, OWN, 0, me, 0, sz).wait_send()

        def sized(r, fn):
            lax.switch((r >> 1) - 1,
                       [functools.partial(fn, s) for s in range(2, C + 1, 2)])

        def loop(lo, hi, fn):
            def b(k, c):
                fn(k)
                return c
            lax.fori_loop(lo, hi, b, 0)

        def send_l(k, sz=C):
            rcopy(OWN, FROM_R, k, left, M - 1 - k, sz).start()

        def send_r(k, sz=C):
            rcopy(OWN, FROM_L, k, right, k, sz).start()

        def catch_up(n):
            pl.semaphore_wait(rdy, 1)

            @pl.when(me == 3)
            def _():
                loop(0, n, send_l)

            @pl.when(me == 1)
            def _():
                loop(0, n, send_r)

        def issue_gather(k):
            for r in range(C):
                row = lst[k * C + r] & (V - 1)
                pltpu.make_async_copy(
                    tab_ref.at[pl.ds(row, 1)],
                    gbuf.at[k, pl.ds(r, 1)], gsem.at[k & (NG - 1)]).start()

        def pack(k):
            pltpu.make_async_copy(gbuf.at[k], gbuf.at[k], gsem.at[k & (NG - 1)]).wait()
            xb = pltpu.bitcast(
                gbuf[k].astype(jnp.bfloat16).astype(jnp.float32), jnp.uint32)
            w = xb[:, :H] | (xb[:, H:] >> 16)
            pbuf[pl.ds(chunk_start(OWN, k), 4 * C), :] = w.reshape(4 * C, 128)

            @pl.when(k == 0)
            def _():
                @pl.when(me == 0)
                def _():
                    pl.semaphore_wait(bar, 2)

                @pl.when(is_mid)
                def _():
                    pl.semaphore_wait(bar, 1)

        def pack_send(k):
            pack(k)

            @pl.when((k == K0) & is_mid)
            def _():
                catch_up(K0)

            @pl.when((k >= K0) | (me != 3))
            def _():
                send_l(k)

            @pl.when((k >= K0) | (me != 1))
            def _():
                send_r(k)

        def find_repeats():
            cp_v.wait()
            idxv = idx_v[...] & (N_DEV * V - 1)
            pos = (lax.broadcasted_iota(jnp.int32, (NB, 128), 0) * 128
                   + lax.broadcasted_iota(jnp.int32, (NB, 128), 1))
            sub = lax.broadcasted_iota(jnp.int32, (8, 128), 0)
            idx_t = idxv.T
            rows = {pb: jnp.broadcast_to(idxv[pb:pb + 1, :], (8, 128))
                    for pb in range(PB0, NB)}
            acc = {pb: jnp.full((8, 128), N, jnp.int32) for pb in range(PB0, NB)}
            for b in range(NB - 1, -1, -1):
                xb = jnp.broadcast_to(idx_t[:, b:b + 1], (128, 128))
                for u in range(15, -1, -1):
                    xq = xb[8 * u:8 * u + 8]
                    qv = sub + (128 * b + 8 * u)
                    for pb in range(max(b, PB0), NB):
                        acc[pb] = lax.select(lax.eq(xq, rows[pb]), qv, acc[pb])
            first = jnp.concatenate(
                [pos[0:PB0]]
                + [jnp.min(acc[pb], axis=0, keepdims=True) for pb in range(PB0, NB)],
                axis=0)
            rel = jnp.where(first == pos, ((idxv >> LV) - me) & 3, N_DEV)
            row_v[...] = jnp.where(rel == OWN, (idxv & (V - 1)) - V, 0).reshape(N)
            cp_row.start()
            first_v[...] = first.reshape(N)
            cp_first.start()
            idx_v[...] = rel

        def find_slots():
            rel = idx_v[...]
            row = lax.broadcasted_iota(jnp.int32, (NB, 128), 0)
            lane = lax.broadcasted_iota(jnp.int32, (NB, 128), 1)
            inc = jnp.zeros((NB, 128), jnp.int32)
            for o in range(N_DEV):
                inc = jnp.where(rel == o, 1 << (8 * o), inc)
            for sh in (1, 2, 4, 8, 16, 32, 64):
                inc = inc + jnp.where(lane >= sh, pltpu.roll(inc, sh, 1), 0)
            tot = jnp.broadcast_to(inc[:, 127:128], (NB, 128))
            upto = []
            for h in range(2):
                t = lax.shift_right_logical(tot, 8 * h) & 0x00FF00FF
                acc = t
                for sh in (1, 2, 4, 8):
                    acc = acc + jnp.where(row >= sh, pltpu.roll(acc, sh, 0), 0)
                upto.append((acc - t, acc))
            sub = lax.broadcasted_iota(jnp.int32, (8, 128), 0)
            slot = jnp.zeros((NB, 128), jnp.int32)
            lens = jnp.zeros((8, 128), jnp.int32)
            for o in range(N_DEV):
                before, after = [(x >> (16 * (o >> 1))) & 0xFFFF for x in upto[o & 1]]
                rank = before + (lax.shift_right_logical(inc, 8 * o) & 0xFF)
                slot = jnp.where(rel == o, (rank + (o * N - 1)) * 4, slot)
                lens = jnp.where(
                    sub == o, jnp.broadcast_to(after[NB - 1:NB], (8, 128)), lens)
                if o == DIAG:
                    meta_v[0:NB, :] = jnp.maximum((rank + (C - 1)) >> LC, 1)
            slot_v[...] = slot.reshape(N)
            cp_slot.start()
            meta_v[NB:NB + 8, :] = jnp.maximum((lens + 1) & -2, 2)
            cp_meta.start()

        base = me * V

        def step(raw, t, carry):
            cnt, issued, before, sent = carry
            if raw:
                @pl.when(t == I0 // S)
                def _():
                    cp_s1.wait()

                @pl.when(t == TB)
                def _():
                    find_repeats()
            for i in range(S):
                if raw:
                    v = ((idx_s[t * S + i] - base) & (N_DEV * V - 1)) - V
                else:
                    v = row_s[t * S + i]
                lst[cnt] = v
                cnt = cnt + lax.shift_right_logical(v, 31)
            new_issued = cnt >> LC
            loop(issued, new_issued, issue_gather)
            ready = jnp.where(t == TB - 1, issued, before) if raw else before
            new_sent = jnp.maximum(sent, jnp.minimum(ready, new_issued - 1))
            loop(sent, new_sent, pack_send)
            return cnt, new_issued, issued, new_sent

        carry = lax.fori_loop(0, P0 // S, functools.partial(step, True),
                              (jnp.int32(0),) * 4)
        cp_row.wait()
        cnt, issued, _, sent = lax.fori_loop(
            P0 // S, N // S, functools.partial(step, False), carry)
        for i in range(C):
            lst[cnt + i] = 0
        c_me = jnp.maximum((cnt + 1) & -2, 2)
        n_me = (c_me + C - 1) >> LC
        loop(issued, n_me, issue_gather)
        find_slots()

        k_me = n_me - 1
        r_me = c_me - (k_me << LC)
        loop(sent, k_me, pack_send)
        pack(k_me)

        @pl.when((k_me <= K0) & is_mid)
        def _():
            catch_up(k_me)

        def send_last(sz):
            send_l(k_me, sz)
            send_r(k_me, sz)
        sized(r_me, send_last)

        cp_first.wait()
        cp_slot.wait()
        cp_meta.wait()

        c_l, c_r, c_d = meta_s[NB + FROM_L, 0], meta_s[NB + FROM_R, 0], meta_s[NB + DIAG, 0]
        k_l, k_r, k_d = (c_l - 1) >> LC, (c_r - 1) >> LC, (c_d - 1) >> LC
        r_l, r_r, r_d = c_l - (k_l << LC), c_r - (k_r << LC), c_d - (k_d << LC)
        n_l, n_d = k_l + 1, k_d + 1

        def via_left(k, d):
            return (k < d) | ((k >= jnp.abs(d)) & (((k + d) & 1) == 0))

        x = c_me - c_d + jnp.where(me == 0, -HEAD, jnp.where(me == 2, HEAD, 0))
        d1 = (-x) >> LC
        d2 = x >> LC
        fwd_last_l = via_left(k_l, d1)
        fwd_last_r = jnp.logical_not(via_left(k_r, d2))

        def fwd_l(k, sz=C):
            rcopy(FROM_L, DIAG, k, right, n_me + k, sz).start()

        def fwd_r(k, sz=C):
            rcopy(FROM_R, DIAG, k, left, n_d + k, sz).start()

        def fwd(k, nf):
            f1 = (k < k_l) & via_left(k, d1)
            f2 = (k < k_r) & jnp.logical_not(via_left(k, d2))

            @pl.when(k < k_l)
            def _():
                wait_recv(FROM_L, k, k)

            @pl.when(f1)
            def _():
                fwd_l(k)

            @pl.when(k < k_r)
            def _():
                wait_recv(FROM_R, k, M - 1 - k)

            @pl.when(f2)
            def _():
                fwd_r(k)
            return nf + f1.astype(jnp.int32) + f2.astype(jnp.int32)

        n_f = lax.fori_loop(0, jnp.maximum(k_l, k_r), fwd, jnp.int32(0))

        def last_l(sz):
            wait_recv(FROM_L, k_l, k_l, sz)

            @pl.when(fwd_last_l)
            def _():
                fwd_l(k_l, sz)

        def last_r(sz):
            wait_recv(FROM_R, k_r, M - 1 - k_r, sz)

            @pl.when(fwd_last_r)
            def _():
                fwd_r(k_r, sz)

        sized(r_l, last_l)
        sized(r_r, last_r)

        n_s = n_f + 2 * k_me

        def wait_send2(sz):
            wait_send(sz=sz)
            wait_send(sz=sz)
        sized(r_me, wait_send2)

        @pl.when(fwd_last_l)
        def _():
            sized(r_l, lambda sz: wait_send(sz=sz))

        @pl.when(fwd_last_r)
        def _():
            sized(r_r, lambda sz: wait_send(sz=sz))

        def wait_diag(have, need):
            loop(have, jnp.minimum(need, k_d), lambda k: wait_recv(DIAG, k, n_l + k))

            @pl.when((need == n_d) & (have < n_d))
            def _():
                sized(r_d, lambda sz: wait_recv(DIAG, k_d, n_l + k_d, sz))

        def blk(b, carry):
            have, done = carry
            for g in range(128 // G):
                c0 = g * G
                need = meta_s[b, c0 + G - 1]
                wait_diag(have, need)
                have = need
                p0 = pl.multiple_of(b * 128 + c0, G)
                rows = [pbuf[pl.ds(pl.multiple_of(slot_s[first_s[p0 + r]], 4), 4), :]
                        for r in range(G)]
                w = jnp.concatenate(
                    [jnp.concatenate([x[j:j + 1, :] for x in rows], axis=0)
                     for j in range(4)], axis=1)
                hi = pltpu.bitcast(w & jnp.uint32(0xFFFF0000), jnp.float32)
                lo = pltpu.bitcast(w << 16, jnp.float32)
                out_ref[pl.ds(p0, G), 0:H] = hi.astype(out_ref.dtype)
                out_ref[pl.ds(p0, G), H:D] = lo.astype(out_ref.dtype)
                if g == 1:
                    tgt = n_s - KEEP - ((n_f * (NB - 1 - b)) >> 3)
                    loop(done, tgt, wait_send)
                    done = jnp.maximum(tgt, done)
            return have, done

        _, done = lax.fori_loop(0, NB, blk, (jnp.int32(0), jnp.int32(0)))
        loop(done, n_s, wait_send)

    return pl.pallas_call(
        body,
        out_shape=jax.ShapeDtypeStruct((N, D), jnp.bfloat16),
        in_specs=[pl.BlockSpec(memory_space=pl.ANY)] * 3,
        out_specs=pl.BlockSpec(memory_space=pltpu.VMEM),
        scratch_shapes=[
            pltpu.SMEM((P0,), jnp.int32),
            pltpu.SMEM((N + C,), jnp.int32),
            pltpu.SMEM((N,), jnp.int32),
            pltpu.SMEM((N,), jnp.int32),
            pltpu.SMEM((N,), jnp.int32),
            pltpu.SMEM((NB + 8, 128), jnp.int32),
            pltpu.VMEM((NB, 128), jnp.int32),
            pltpu.VMEM((N,), jnp.int32),
            pltpu.VMEM((N,), jnp.int32),
            pltpu.VMEM((N,), jnp.int32),
            pltpu.VMEM((NB + 8, 128), jnp.int32),
            pltpu.VMEM((NCH, C, D), jnp.float32),
            pltpu.VMEM((N_DEV * N * 4, 128), jnp.uint32),
            pltpu.SemaphoreType.DMA((7,)),
            pltpu.SemaphoreType.DMA((NG,)),
            pltpu.SemaphoreType.DMA,
            pltpu.SemaphoreType.DMA((M,)),
            pltpu.SemaphoreType.REGULAR,
        ],
        compiler_params=pltpu.CompilerParams(
            collective_id=0, vmem_limit_bytes=64 << 20,
            disable_bounds_checks=True, disable_semaphore_checks=True),
    )(idx, idx2, table)
```
